```python
import numpy as np

kernel_name = "dist_moe_top2_ep_n2048_d512_e4_h1024"

def setup_inputs():
    x = np.random.randn(2048, 512).astype(np.float32)
    router_W = np.random.randn(512, 16).astype(np.float32) * 0.1
    scores64 = x.astype(np.float64) @ router_W.astype(np.float64)
    route_idx = np.argsort(-scores64, axis=-1)[:, :2].astype(np.int32)
    expert_W = np.random.randn(16, 512, 1024).astype(np.float32) * 0.02
    return {"x": x, "router_W": router_W, "route_idx": route_idx, "expert_W": expert_W}

def reference(x, router_W, route_idx, expert_W):
    scores = x @ router_W
    s_max = scores.max(axis=-1, keepdims=True)
    probs = np.exp(scores - s_max)
    probs = probs / probs.sum(axis=-1, keepdims=True)
    out = np.zeros((2048, 1024), dtype=np.float32)
    for i in range(2048):
        e0, e1 = int(route_idx[i, 0]), int(route_idx[i, 1])
        g0, g1 = probs[i, e0], probs[i, e1]
        gs = g0 + g1
        out[i] = (g0 / gs) * (x[i] @ expert_W[e0]) + (g1 / gs) * (x[i] @ expert_W[e1])
    return out
```

```python
import jax
import jax.numpy as jnp
from jax import lax
from jax.experimental import pallas as pl
from jax.experimental.pallas import tpu as pltpu

N_TOK, D, H = 2048, 512, 1024
N_DEV, E_LOC, N_EXP = 4, 4, 16
T = 128
NB = N_TOK // T
S = T // N_DEV
TM = 144
CAP = 2160
ARR0 = E_LOC * CAP
N_ROWS = ARR0 + 2 * NB * S
N_BITS = 10
XCH = 4
XR = N_TOK // XCH
L1, L2 = 1, 2

f32, bf16, i32 = jnp.float32, jnp.bfloat16, jnp.int32
MESH = pl.DeviceIdType.MESH


def _iota(shape, dim):
    return lax.broadcasted_iota(i32, shape, dim)


def _b2f(mask):
    return jnp.where(mask, 1.0, 0.0).astype(f32)


def _mm(a, b):
    return jnp.dot(a.astype(bf16), b.astype(bf16), preferred_element_type=f32)


def _spread(v):
    blk = _iota((NB, N_TOK), 0) == (_iota((NB, N_TOK), 1) >> 7)
    if v.shape[1] == T:
        v = jnp.concatenate([v] * NB, axis=1)
    else:
        v = jnp.broadcast_to(v, (NB, N_TOK))
    return jnp.where(blk, v, 0.0)


def _ownership(r_v, perm_v):
    e0 = r_v[pl.ds(0, NB, stride=2), :]
    e1 = r_v[pl.ds(1, NB, stride=2), :]
    lane = _iota((NB, T), 1)
    c0, c1 = e0 >> 2, e1 >> 2
    nondiag = ((c1 - c0) & 3) != 2
    pref = jnp.where((lane & 1) == 0, c0, c1)
    r128, c128 = _iota((T, T), 0), _iota((T, T), 1)
    upper = _b2f(r128 < c128)
    ms = [_b2f(jnp.logical_and(pref == c, nondiag)) for c in range(N_DEV)]
    r1 = _mm(jnp.concatenate(ms, axis=0),
             jnp.concatenate([upper, jnp.ones((T, T), f32)], axis=1))
    rank = sum(ms[c] * r1[c * NB:(c + 1) * NB, :T] for c in range(N_DEV))
    used = [jnp.minimum(r1[c * NB:(c + 1) * NB, T:], float(S)) for c in range(N_DEV)]
    accepted = jnp.logical_and(nondiag, rank < float(S))
    q = _mm(_b2f(jnp.logical_not(accepted)), upper)
    cum1 = S - used[0]
    cum2 = cum1 + (S - used[1])
    cum3 = cum2 + (S - used[2])
    base = jnp.where(
        q >= cum3, 3 * S + used[3] - cum3,
        jnp.where(q >= cum2, 2 * S + used[2] - cum2,
                  jnp.where(q >= cum1, S + used[1] - cum1, used[0])))
    slot = jnp.where(accepted, pref.astype(f32) * S + rank, base + q)
    slot_t = jnp.transpose(jnp.concatenate([slot] * (T // NB), axis=0))
    c128f = c128.astype(f32)
    for b in range(NB):
        perm_v[b * T:(b + 1) * T, :] = _b2f(slot_t[:, b:b + 1] == c128f).astype(bf16)
    lhs = jnp.concatenate([_spread(lane.astype(f32)), _spread(e0.astype(f32)),
                           _spread(e1.astype(f32))], axis=0)
    inv = jnp.dot(lhs.astype(bf16), perm_v[...], preferred_element_type=f32)
    toks = inv[0:NB].astype(i32) + (_iota((NB, T), 0) << 7)
    return toks, inv[NB:2 * NB], inv[2 * NB:3 * NB]


def _ranks(e0s, e1s, rank_v):
    r128, c128 = _iota((T, T), 0), _iota((T, T), 1)
    erow = (_iota((N_EXP * NB, T), 0) >> 4).astype(f32)
    mask = _b2f(jnp.logical_or(jnp.concatenate([e0s] * N_EXP, axis=0) == erow,
                               jnp.concatenate([e1s] * N_EXP, axis=0) == erow))
    seg = (r128 >> 5) == (c128 >> 5)
    r2 = _mm(mask, jnp.concatenate([_b2f(jnp.logical_and(seg, r128 < c128)), _b2f(seg)], axis=1))
    tot = r2[:, T:]
    lower = _b2f(jnp.logical_and((r128 >> 4) == (c128 >> 4), c128 < r128))
    pre = jnp.concatenate([_mm(lower, tot[0:T]), _mm(lower, tot[T:2 * T])], axis=0)
    rank_v[...] = r2[:, :T] + pre
    sel = _b2f((_iota((N_EXP, N_EXP * NB), 1) >> 4) == _iota((N_EXP, N_EXP * NB), 0))
    return _mm(sel, tot).astype(i32)


def _offsets(cnt):
    row, lane = _iota((N_EXP, T), 0), _iota((N_EXP, T), 1)
    remote = (row >> 2) != (lane >> 5)
    cm = jnp.where(remote, cnt, 0)
    acc = cm
    for sh in (1, 2, 4, 8):
        acc = acc + jnp.where(row >= sh, pltpu.roll(acc, sh, 0), 0)
    arr = acc - cm
    away = cm + pltpu.roll(cm, S, 1) + pltpu.roll(cm, 2 * S, 1) + pltpu.roll(cm, 3 * S, 1)
    base = jnp.where(remote, ARR0 + arr, (row & 3) * CAP + away)
    return arr, base


def _sender_lists(me, toks, e0s, e1s, rank_v):
    rows = E_LOC * NB
    lane, row = _iota((rows, T), 1), _iota((rows, T), 0)
    ej = (me * E_LOC + (row >> 4)).astype(f32)
    m = jnp.logical_or(jnp.concatenate([e0s] * E_LOC, axis=0) == ej,
                       jnp.concatenate([e1s] * E_LOC, axis=0) == ej)
    rk = rank_v[pl.ds(pl.multiple_of(me * rows, rows), rows), :].astype(i32)
    li = lane & (S - 1)
    d = ((row & (NB - 1)) << 5) + li - rk
    v = jnp.where(m, (jnp.concatenate([toks] * E_LOC, axis=0) << 2) | (d << 13), 0)
    for k in range(5):
        sh, bit = 1 << k, 1 << (13 + k)
        w = jnp.where(li < sh, pltpu.roll(v, rows - 1, 0), v)
        s = jnp.where(li + sh < S, pltpu.roll(w, T - sh, 1), pltpu.roll(w, S - sh, 1))
        v = jnp.where((s & bit) != 0, s, jnp.where((v & bit) != 0, 0, v))
    for k in range(5, 9):
        bit = 1 << (13 + k)
        s = pltpu.roll(v, rows - (1 << (k - 5)), 0)
        v = jnp.where((s & bit) != 0, s, jnp.where((v & bit) != 0, 0, v))
    return v & 0x1FFF


def _owner_addresses(e0s, e1s, base, rank_v):
    basef = base.astype(f32)
    a0 = jnp.zeros((NB, T), f32)
    a1 = jnp.zeros((NB, T), f32)
    for e in range(N_EXP):
        val = rank_v[e * NB:(e + 1) * NB, :] + basef[e:e + 1, :]
        a0 = jnp.where(e0s == float(e), val, a0)
        a1 = jnp.where(e1s == float(e), val, a1)
    return (a0.astype(i32) << 2) | (a1.astype(i32) << 18)


def _pack(lo, hi):
    lo = lax.bitcast_convert_type(lo, i32) + 0x8000
    hi = lax.bitcast_convert_type(hi, i32) + 0x8000
    return (hi & -65536) | lax.shift_right_logical(lo, 16)


def _for_bits(n, fn):
    def one(k):
        @pl.when(((n >> k) & 1) == 1)
        def _():
            fn(k, (n >> (k + 1)) << (k + 1))

    @pl.when(n >= 128)
    def _():
        for k in range(N_BITS - 1, 6, -1):
            one(k)

    for k in range(6, -1, -1):
        one(k)


def _body(r_hbm, rw_hbm, x_hbm, w_hbm, out_hbm,
          r_v, rw_v, x_v, xlin_v, xs_v, w_v, rows_v, f_v, o_v, perm_v, rank_v,
          stmp_v, wrow_v, lst_v, cnt_v, adr_v, gat_v,
          lst_s, cnt_s, adr_s, gat_s,
          ld_sem, sm_sem, rs_send, rs_recv, ag_send, ag_recv, out_sem):
    me = lax.axis_index("i")
    right, diag, left = (me + 1) % N_DEV, (me + 2) % N_DEV, (me + 3) % N_DEV

    r_cp = pltpu.make_async_copy(r_hbm, r_v, ld_sem.at[0])
    rw_cp = pltpu.make_async_copy(rw_hbm, rw_v, ld_sem.at[1])

    def x_cp(q):
        return pltpu.make_async_copy(x_hbm.at[pl.ds(q * XR, XR)], x_v.at[pl.ds(q * XR, XR)],
                                     ld_sem.at[2 + q])

    def w_cp(j):
        return pltpu.make_async_copy(w_hbm.at[j], w_v.at[j], ld_sem.at[2 + XCH + j])

    r_cp.start()
    rw_cp.start()
    for q in range(XCH):
        x_cp(q).start()
    for j in range(E_LOC):
        w_cp(j).start()

    barrier = pltpu.get_barrier_semaphore()
    for peer in (right, diag, left):
        pl.semaphore_signal(barrier, 1, device_id=(peer,), device_id_type=MESH)

    def lst_cp(j):
        return pltpu.make_async_copy(lst_v.at[pl.ds(j * NB, NB)], lst_s.at[pl.ds(j * NB, NB)],
                                     sm_sem.at[j])

    cnt_cp = pltpu.make_async_copy(cnt_v, cnt_s, sm_sem.at[4])
    adr_cp = pltpu.make_async_copy(adr_v, adr_s, sm_sem.at[5])
    gat_cp = pltpu.make_async_copy(gat_v, gat_s, sm_sem.at[6])

    r_cp.wait()
    toks, e0s, e1s = _ownership(r_v, perm_v)
    cnt = _ranks(e0s, e1s, rank_v)
    arr, base = _offsets(cnt)
    cnt_v[...] = jnp.where((_iota((N_EXP, T), 1) & (S - 1)) == 1, arr, cnt)
    cnt_cp.start()
    lst_v[...] = _sender_lists(me, toks, e0s, e1s, rank_v)
    for j in range(E_LOC):
        lst_cp(j).start()
    adr_v[...] = _owner_addresses(e0s, e1s, base, rank_v)
    adr_cp.start()

    rw_cp.wait()
    rw = rw_v[...].astype(bf16)

    def x_chunk(q, carry):
        x_cp(q).wait()
        t0 = pl.multiple_of(q * XR, XR)

        def relayout(i, c):
            r0 = pl.multiple_of(t0 + i * 64, 64)
            for p in range(4):
                xlin_v[pl.ds(r0 * 4 + p, 64, stride=4), :] = x_v[pl.ds(r0, 64), p * 128:(p + 1) * 128]
            return c
        lax.fori_loop(0, XR // 64, relayout, 0)

        s = lax.dot_general(rw, x_v[pl.ds(t0, XR), :].astype(bf16), (((1,), (1,)), ((), ())),
                            preferred_element_type=f32)
        p = jnp.exp(s - jnp.max(s, axis=0, keepdims=True))
        p = p / jnp.sum(p, axis=0, keepdims=True)
        nb = XR // T
        e0 = jnp.concatenate([r_v[pl.ds(2 * (q * nb + b), 1), :] for b in range(nb)], axis=1)
        e1 = jnp.concatenate([r_v[pl.ds(2 * (q * nb + b) + 1, 1), :] for b in range(nb)], axis=1)
        erow = _iota((N_EXP, XR), 0)
        g0 = jnp.sum(jnp.where(erow == e0, p, 0.0), axis=0, keepdims=True)
        g1 = jnp.sum(jnp.where(erow == e1, p, 0.0), axis=0, keepdims=True)
        gs = g0 + g1
        wrow_v[0, pl.ds(q, 1), :] = g0 / gs
        wrow_v[1, pl.ds(q, 1), :] = g1 / gs
        return carry
    lax.fori_loop(0, XCH, x_chunk, 0)

    parts = []
    for k in range(2):
        w = jnp.concatenate([wrow_v[k, q:q + 1, :] for q in range(XCH)], axis=1)
        hi = w.astype(bf16).astype(f32)
        parts += [_spread(hi), _spread(w - hi)]
    g = jnp.dot(jnp.concatenate(parts, axis=0).astype(bf16), perm_v[...], preferred_element_type=f32)
    gat_v[0:NB, :] = g[0:NB] + g[NB:2 * NB]
    gat_v[NB:2 * NB, :] = g[2 * NB:3 * NB] + g[3 * NB:4 * NB]
    gat_cp.start()

    cnt_cp.wait()
    pl.semaphore_wait(barrier, N_DEV - 1)

    dests = ((right, 2), (left, 0), (diag, 1))

    def rs_copy(j, k, src_row, dst_row, dev, rel):
        n = 4 << k
        return pltpu.make_async_remote_copy(
            src_ref=rows_v.at[pl.ds(src_row * 4, n)], dst_ref=rows_v.at[pl.ds(dst_row * 4, n)],
            send_sem=rs_send, recv_sem=rs_recv.at[(rel * E_LOC + j) * N_BITS + k],
            device_id=(dev,), device_id_type=MESH)

    def for_rs_sends(j, action):
        e = me * E_LOC + j
        off = j * CAP
        for dev, rel in dests:
            n = cnt_s[e, dev * S]
            dst = ARR0 + cnt_s[e, dev * S + 1]
            _for_bits(n, lambda k, o, off=off, dst=dst, dev=dev, rel=rel:
                      action(rs_copy(j, k, off + o, dst + o, dev, rel)))
            off = off + n

    def expert(j, carry):
        e = me * E_LOC + j
        lst_cp(j).wait()
        off = 0
        for dev in (right, left, diag, me):
            n = cnt_s[e, dev * S]

            def gather(m, c, off=off, dev=dev):
                row = j * NB + (m >> 2)
                col = dev * S + (m & 3) * 8
                for u in range(8):
                    a = pl.multiple_of(lst_s[row, col + u], 4)
                    xs_v[pl.ds(pl.multiple_of((off + m * 8 + u) * 4, 4), 4), :] = xlin_v[pl.ds(a, 4), :]
                return c
            lax.fori_loop(0, (n + 7) >> 3, gather, 0)
            if dev is diag:
                n_away = off + n
            off = off + n
        last_away = (n_away + TM - 1) // TM - 1
        w_cp(j).wait()

        def tile(t, c):
            r0 = pl.multiple_of(t * TM, 16)
            lhs = jnp.concatenate([xs_v[pl.ds(r0 * 4 + p, TM, stride=4), :] for p in range(4)], axis=1)
            y = jnp.dot(lhs.astype(bf16), w_v[j].astype(bf16), preferred_element_type=f32)
            for p in range(4):
                rows_v[pl.ds((j * CAP + r0) * 4 + p, TM, stride=4), :] = _pack(
                    y[:, p * 128:(p + 1) * 128], y[:, 512 + p * 128:512 + (p + 1) * 128])

            @pl.when(t == last_away)
            def _():
                for_rs_sends(j, lambda cp: cp.start())
            return c
        lax.fori_loop(0, (off + TM - 1) // TM, tile, 0)
        return carry
    lax.fori_loop(0, E_LOC, expert, 0)

    def rs_wait(j, carry):
        for rel in range(N_DEV - 1):
            src = (me + 1 + rel) % N_DEV
            e = src * E_LOC + j
            dst = ARR0 + cnt_s[e, me * S + 1]
            _for_bits(cnt_s[e, me * S], lambda k, o, dst=dst, src=src, rel=rel:
                      rs_copy(j, k, dst + o, dst + o, src, rel).wait_recv())
        return carry
    lax.fori_loop(0, E_LOC, rs_wait, 0)
    adr_cp.wait()
    gat_cp.wait()

    def f_rows(b, owner, start, n):
        return f_v.at[pl.ds(pl.multiple_of(b * T + owner * S + start, 16), n)]

    def ag_copy(b, kind):
        owner, start, n, dev = ((me, 0, S, right), (me, 0, S, left),
                                (left, 0, S // 2, right), (right, S // 2, S // 2, left))[kind]
        ref = f_rows(b, owner, start, n)
        return pltpu.make_async_remote_copy(
            src_ref=ref, dst_ref=ref, send_sem=ag_send.at[kind], recv_sem=ag_recv.at[b * 4 + kind],
            device_id=(dev,), device_id_type=MESH)

    def ag_arrival(b, kind):
        owner, start, n, dev = ((left, 0, S, left), (right, 0, S, right),
                                (diag, 0, S // 2, left), (diag, S // 2, S // 2, right))[kind]
        ref = f_rows(b, owner, start, n)
        return pltpu.make_async_remote_copy(
            src_ref=ref, dst_ref=ref, send_sem=ag_send.at[kind], recv_sem=ag_recv.at[b * 4 + kind],
            device_id=(dev,), device_id_type=MESH)

    def out_cp(b):
        rows = pl.ds(pl.multiple_of(b * T, T), T)
        return pltpu.make_async_copy(o_v.at[rows], out_hbm.at[rows], out_sem.at[b])

    def step(i, carry):
        @pl.when(i < NB)
        def _():
            def slots(m, c):
                for u in range(8):
                    s = m * 8 + u
                    a = adr_s[i, me * S + s]
                    g0 = gat_s[i, me * S + s]
                    g1 = gat_s[NB + i, me * S + s]
                    r0 = rows_v[pl.ds(pl.multiple_of(a & 0xFFFF, 4), 4), :]
                    r1 = rows_v[pl.ds(pl.multiple_of(lax.shift_right_logical(a, 16), 4), 4), :]
                    lo = (lax.bitcast_convert_type(r0 << 16, f32) * g0
                          + lax.bitcast_convert_type(r1 << 16, f32) * g1)
                    hi = (lax.bitcast_convert_type(r0 & -65536, f32) * g0
                          + lax.bitcast_convert_type(r1 & -65536, f32) * g1)
                    stmp_v[pl.ds(pl.multiple_of(s * 8, 8), 4), :] = lo
                    stmp_v[pl.ds(pl.multiple_of(s * 8 + 4, 4), 4), :] = hi
                return c
            lax.fori_loop(0, S // 8, slots, 0)
            mine = pl.ds(pl.multiple_of(i * T + me * S, S), S)
            for c in range(8):
                f_v[mine, c * 128:(c + 1) * 128] = stmp_v[pl.ds(c, S, stride=8), :].astype(bf16)
            ag_copy(i, 0).start()
            ag_copy(i, 1).start()

        @pl.when(jnp.logical_and(i >= L1, i < NB + L1))
        def _():
            b = i - L1
            ag_arrival(b, 0).wait_recv()
            ag_copy(b, 2).start()
            ag_arrival(b, 1).wait_recv()
            ag_copy(b, 3).start()

        @pl.when(i >= L2)
        def _():
            b = i - L2
            ag_arrival(b, 2).wait_recv()
            ag_arrival(b, 3).wait_recv()
            rows = pl.ds(pl.multiple_of(b * T, T), T)
            o_v[rows, :] = jnp.dot(perm_v[rows, :], f_v[rows, :], preferred_element_type=f32)
            out_cp(b).start()
        return carry
    lax.fori_loop(0, NB + L2, step, 0)

    def drain_rs(j, carry):
        for_rs_sends(j, lambda cp: cp.wait_send())
        return carry
    lax.fori_loop(0, E_LOC, drain_rs, 0)

    def drain(b, carry):
        for kind in range(4):
            ag_copy(b, kind).wait_send()
        out_cp(b).wait()
        return carry
    lax.fori_loop(0, NB, drain, 0)


def pallas_dist_moe_top2_ep_n2048_d512_e4_h1024_kernel(
    x: jax.Array,
    router_W: jax.Array,
    route_idx: jax.Array,
    expert_W: jax.Array,
):
    r = route_idx.astype(i32).reshape(NB, T, 2).transpose(0, 2, 1).reshape(2 * NB, T)
    any_spec = pl.BlockSpec(memory_space=pl.ANY)
    return pl.pallas_call(
        _body,
        out_shape=jax.ShapeDtypeStruct((N_TOK, H), f32),
        in_specs=[any_spec] * 4,
        out_specs=any_spec,
        scratch_shapes=[
            pltpu.VMEM((2 * NB, T), i32),
            pltpu.VMEM((N_EXP, D), f32),
            pltpu.VMEM((N_TOK, D), f32),
            pltpu.VMEM((N_TOK * 4, 128), f32),
            pltpu.VMEM((CAP * 4, 128), f32),
            pltpu.VMEM((E_LOC, D, H), f32),
            pltpu.VMEM((N_ROWS * 4, 128), i32),
            pltpu.VMEM((N_TOK, H), bf16),
            pltpu.VMEM((N_TOK, H), f32),
            pltpu.VMEM((N_TOK, T), bf16),
            pltpu.VMEM((N_EXP * NB, T), f32),
            pltpu.VMEM((S * 8, 128), f32),
            pltpu.VMEM((2, 8, XR), f32),
            pltpu.VMEM((E_LOC * NB, T), i32),
            pltpu.VMEM((N_EXP, T), i32),
            pltpu.VMEM((NB, T), i32),
            pltpu.VMEM((2 * NB, T), f32),
            pltpu.SMEM((E_LOC * NB, T), i32),
            pltpu.SMEM((N_EXP, T), i32),
            pltpu.SMEM((NB, T), i32),
            pltpu.SMEM((2 * NB, T), f32),
            pltpu.SemaphoreType.DMA((2 + XCH + E_LOC,)),
            pltpu.SemaphoreType.DMA((7,)),
            pltpu.SemaphoreType.DMA,
            pltpu.SemaphoreType.DMA(((N_DEV - 1) * E_LOC * N_BITS,)),
            pltpu.SemaphoreType.DMA((4,)),
            pltpu.SemaphoreType.DMA((NB * 4,)),
            pltpu.SemaphoreType.DMA((NB,)),
        ],
        compiler_params=pltpu.CompilerParams(
            collective_id=0, vmem_limit_bytes=100 * 1024 * 1024),
    )(r, router_W.T, x, expert_W)
```

```python
import jax
import jax.numpy as jnp
from jax import lax
from jax.experimental import pallas as pl
from jax.experimental.pallas import tpu as pltpu

N_TOK, D, H = 2048, 512, 1024
N_DEV, E_LOC, N_EXP = 4, 4, 16
T = 128
NB = N_TOK // T
S = T // N_DEV
HB = NB // 2
TM = 160
CAP = N_TOK + TM
XS_CAP = -(-(N_TOK // 2) // TM) * TM
ARR0 = E_LOC * CAP
N_ROWS = ARR0 + 2 * NB * S
CH_BITS = 4
CH = 1 << CH_BITS
N_CH = 2 * NB * S // CH
N_REM = 4
HELD = 2 * E_LOC - 3
EARLY = 2
XCH = 4
XR = N_TOK // XCH
L1, L2 = 1, 3

f32, bf16, i32 = jnp.float32, jnp.bfloat16, jnp.int32
MESH = pl.DeviceIdType.MESH


def _iota(shape, dim):
    return lax.broadcasted_iota(i32, shape, dim)


def _b2f(mask):
    return jnp.where(mask, 1.0, 0.0).astype(f32)


def _mm(a, b):
    return jnp.dot(a.astype(bf16), b.astype(bf16), preferred_element_type=f32)


def _spread(v):
    blk = _iota((NB, N_TOK), 0) == (_iota((NB, N_TOK), 1) >> 7)
    return jnp.where(blk, jnp.concatenate([v] * NB, axis=1), 0.0)


def _ownership(r_v, perm_v):
    e0 = r_v[pl.ds(0, NB, stride=2), :]
    e1 = r_v[pl.ds(1, NB, stride=2), :]
    lane = _iota((NB, T), 1)
    c0, c1 = e0 >> 2, e1 >> 2
    diag = ((c1 - c0) & 3) == 2
    j0, j1 = e0 & 3, e1 & 3
    pref = jnp.where(j0 > j1, c0, jnp.where(j1 > j0, c1, jnp.where((lane & 1) == 0, c0, c1)))
    r128, c128 = _iota((T, T), 0), _iota((T, T), 1)
    upper = _b2f(r128 < c128)
    m1 = [_b2f(jnp.logical_and(pref == c, jnp.logical_not(diag))) for c in range(N_DEV)]
    m2 = [_b2f(jnp.logical_and(pref == c, diag)) for c in range(N_DEV)]
    r1 = _mm(jnp.concatenate(m1 + m2, axis=0),
             jnp.concatenate([upper, jnp.ones((T, T), f32)], axis=1))
    part = lambda k: r1[k * NB:(k + 1) * NB]
    rank = sum(m1[c] * part(c)[:, :T]
               + m2[c] * (part(N_DEV + c)[:, :T] + part(c)[:, T:]) for c in range(N_DEV))
    used = [jnp.minimum(part(c)[:, T:] + part(N_DEV + c)[:, T:], float(S)) for c in range(N_DEV)]
    accepted = rank < float(S)
    q = _mm(_b2f(jnp.logical_not(accepted)), upper)
    cum1 = S - used[0]
    cum2 = cum1 + (S - used[1])
    cum3 = cum2 + (S - used[2])
    base = jnp.where(
        q >= cum3, 3 * S + used[3] - cum3,
        jnp.where(q >= cum2, 2 * S + used[2] - cum2,
                  jnp.where(q >= cum1, S + used[1] - cum1, used[0])))
    slot = jnp.where(accepted, pref.astype(f32) * S + rank, base + q)
    slot_t = jnp.transpose(jnp.concatenate([slot] * (T // NB), axis=0))
    c128f = c128.astype(f32)
    for b in range(NB):
        perm_v[b * T:(b + 1) * T, :] = _b2f(slot_t[:, b:b + 1] == c128f).astype(bf16)
    lhs = jnp.concatenate([_spread(lane.astype(f32)), _spread(e0.astype(f32)),
                           _spread(e1.astype(f32))], axis=0)
    inv = jnp.dot(lhs.astype(bf16), perm_v[...], preferred_element_type=f32)
    toks = inv[0:NB].astype(i32) + (_iota((NB, T), 0) << 7)
    return toks, inv[NB:2 * NB], inv[2 * NB:3 * NB]


def _ranks(e0s, e1s, rank_v):
    r128, c128 = _iota((T, T), 0), _iota((T, T), 1)
    erow = (_iota((N_EXP * NB, T), 0) >> 4).astype(f32)
    mask = _b2f(jnp.logical_or(jnp.concatenate([e0s] * N_EXP, axis=0) == erow,
                               jnp.concatenate([e1s] * N_EXP, axis=0) == erow))
    seg = (r128 >> 5) == (c128 >> 5)
    r2 = _mm(mask, jnp.concatenate([_b2f(jnp.logical_and(seg, r128 < c128)), _b2f(seg)], axis=1))
    tot = r2[:, T:]
    lower = _b2f(jnp.logical_and((r128 >> 3) == (c128 >> 3), c128 < r128))
    pre = jnp.concatenate([_mm(lower, tot[0:T]), _mm(lower, tot[T:2 * T])], axis=0)
    rank_v[...] = r2[:, :T] + pre
    srow, scol = _iota((2 * N_EXP, N_EXP * NB), 0), _iota((2 * N_EXP, N_EXP * NB), 1)
    sel = _b2f((scol >> 3) == ((srow & (N_EXP - 1)) << 1) + (srow >> 4))
    cnt = _mm(sel, tot).astype(i32)
    return cnt[:N_EXP], cnt[N_EXP:]


def _offsets(cnt0, cnt1):
    row, lane = _iota((N_EXP, T), 0), _iota((N_EXP, T), 1)
    remote = (row >> 2) != (lane >> 5)
    cm = jnp.where(remote, cnt0 + cnt1, 0)
    acc = cm
    for sh in (1, 2, 4, 8):
        acc = acc + jnp.where(row >= sh, pltpu.roll(acc, sh, 0), 0)
    arr = acc - cm

    def over_owners(v):
        return v + pltpu.roll(v, S, 1) + pltpu.roll(v, 2 * S, 1) + pltpu.roll(v, 3 * S, 1)

    home = (row & 3) * CAP
    base0 = jnp.where(remote, ARR0 + arr, home + over_owners(jnp.where(remote, cnt0, 0)))
    base1 = jnp.where(remote, ARR0 + arr + cnt0,
                      home + over_owners(cnt0 + jnp.where(remote, cnt1, 0)))
    return arr, base0, base1


def _sender_lists(me, toks, e0s, e1s, rank_v):
    rows = E_LOC * NB
    lane, row = _iota((rows, T), 1), _iota((rows, T), 0)
    ej = (me * E_LOC + (row >> 4)).astype(f32)
    m = jnp.logical_or(jnp.concatenate([e0s] * E_LOC, axis=0) == ej,
                       jnp.concatenate([e1s] * E_LOC, axis=0) == ej)
    rk = rank_v[pl.ds(pl.multiple_of(me * rows, rows), rows), :].astype(i32)
    li = lane & (S - 1)
    d = ((row & (HB - 1)) << 5) + li - rk
    v = jnp.where(m, (jnp.concatenate([toks] * E_LOC, axis=0) << 2) | (d << 13), 0)
    for k in range(5):
        sh, bit = 1 << k, 1 << (13 + k)
        w = jnp.where(li < sh, pltpu.roll(v, rows - 1, 0), v)
        s = jnp.where(li + sh < S, pltpu.roll(w, T - sh, 1), pltpu.roll(w, S - sh, 1))
        v = jnp.where((s & bit) != 0, s, jnp.where((v & bit) != 0, 0, v))
    for k in range(5, 8):
        bit = 1 << (13 + k)
        s = pltpu.roll(v, rows - (1 << (k - 5)), 0)
        v = jnp.where((s & bit) != 0, s, jnp.where((v & bit) != 0, 0, v))
    return v & 0x1FFF


def _owner_addresses(e0s, e1s, base0, base1, rank_v):
    base0, base1 = base0.astype(f32), base1.astype(f32)
    first_half = _iota((NB, T), 0) < HB
    a0 = jnp.zeros((NB, T), f32)
    a1 = jnp.zeros((NB, T), f32)
    for e in range(N_EXP):
        val = rank_v[e * NB:(e + 1) * NB, :] + jnp.where(first_half, base0[e:e + 1, :], base1[e:e + 1, :])
        a0 = jnp.where(e0s == float(e), val, a0)
        a1 = jnp.where(e1s == float(e), val, a1)
    return (a0.astype(i32) << 2) | (a1.astype(i32) << 18)


def _pack(lo, hi):
    lo = lax.bitcast_convert_type(lo, i32) + 0x8000
    hi = lax.bitcast_convert_type(hi, i32) + 0x8000
    return (hi & -65536) | lax.shift_right_logical(lo, 16)


def _for_pieces(sizes, fn):
    def chunks(s):
        def chunk(c, carry):
            fn(s, c * CH, CH, None)
            return carry
        lax.fori_loop(0, sizes[s] >> CH_BITS, chunk, 0)

    chunks(0)
    for s, n in enumerate(sizes):
        for k in range(N_REM - 1, -1, -1):
            @pl.when(((n >> k) & 1) == 1)
            def _(s=s, n=n, k=k):
                fn(s, (n >> (k + 1)) << (k + 1), 1 << k, k)
    for s in range(1, len(sizes)):
        chunks(s)


def _body(r_hbm, rw_hbm, x_hbm, w_hbm, o_v,
          r_v, rw_v, x_v, xlin_v, xs_v, w_v, rows_v, f_v, perm_v, rank_v,
          stmp_v, lst_v, cnt_v, adr_v, gat_v,
          lst_s, cnt_s, adr_s, gat_s,
          ld_sem, sm_sem, rs_send, rs_recv, ag_send, ag_recv):
    me = lax.axis_index("i")
    right, diag, left = (me + 1) & 3, (me + 2) & 3, (me + 3) & 3

    r_cp = pltpu.make_async_copy(r_hbm, r_v.at[pl.ds(0, 2 * NB)], ld_sem.at[0])
    rw_cp = pltpu.make_async_copy(rw_hbm, rw_v, ld_sem.at[1])

    def x_cp(q):
        return pltpu.make_async_copy(x_hbm.at[pl.ds(q * XR, XR)], x_v.at[pl.ds(q * XR, XR)],
                                     ld_sem.at[2 + q])

    def w_cp(j):
        return pltpu.make_async_copy(w_hbm.at[j], w_v.at[j], ld_sem.at[2 + XCH + j])

    r_cp.start()
    rw_cp.start()
    for q in range(XCH // 2):
        x_cp(q).start()
    w_cp(0).start()
    for q in range(XCH // 2, XCH):
        x_cp(q).start()
    for j in range(1, E_LOC):
        w_cp(j).start()

    barrier = pltpu.get_barrier_semaphore()
    for peer in (right, diag, left):
        pl.semaphore_signal(barrier, 1, device_id=(peer,), device_id_type=MESH)

    def lst_cp(j):
        return pltpu.make_async_copy(lst_v.at[pl.ds(j * N_TOK, N_TOK)],
                                     lst_s.at[pl.ds(j * N_TOK, N_TOK)], sm_sem.at[j])

    cnt_cp = pltpu.make_async_copy(cnt_v, cnt_s, sm_sem.at[4])
    adr_cp = pltpu.make_async_copy(adr_v, adr_s, sm_sem.at[5])

    r_cp.wait()
    toks, e0s, e1s = _ownership(r_v, perm_v)
    cnt0, cnt1 = _ranks(e0s, e1s, rank_v)
    arr, base0, base1 = _offsets(cnt0, cnt1)
    field = _iota((N_EXP, T), 1) & (S - 1)
    cnt_v[...] = jnp.where(field == 0, cnt0, jnp.where(field == 1, cnt1, arr)).reshape(N_EXP * T)
    cnt_cp.start()
    lst_v[...] = _sender_lists(me, toks, e0s, e1s, rank_v).reshape(E_LOC * N_TOK)
    for j in range(E_LOC):
        lst_cp(j).start()
    adr_v[...] = _owner_addresses(e0s, e1s, base0, base1, rank_v).reshape(N_TOK)
    adr_cp.start()

    def x_chunk(q, carry):
        x_cp(q).wait()
        t0 = pl.multiple_of(q * XR, XR)

        def relayout(i, c):
            r0 = pl.multiple_of(t0 + i * 64, 64)
            for p in range(4):
                xlin_v[pl.ds(r0 * 4 + p, 64, stride=4), :] = x_v[pl.ds(r0, 64), p * 128:(p + 1) * 128]
            return c
        lax.fori_loop(0, XR // 64, relayout, 0)
        return carry

    def gat_cp(h):
        rows = pl.ds(pl.multiple_of(h * N_TOK, N_TOK), N_TOK)
        return pltpu.make_async_copy(gat_v.at[rows], gat_s.at[rows], sm_sem.at[6 + h])

    def gates(h):
        n = N_TOK // 2
        toks = pl.ds(pl.multiple_of(h * n, n), n)
        s = lax.dot_general(rw_v[...].astype(bf16), x_v[toks, :].astype(bf16),
                            (((1,), (1,)), ((), ())), preferred_element_type=f32)
        p = jnp.exp(s - jnp.max(s, axis=0, keepdims=True))
        p = p / jnp.sum(p, axis=0, keepdims=True)
        erow = _iota((N_EXP, n), 0)
        g = []
        for k in range(2):
            e = jnp.concatenate([r_v[pl.ds(2 * (h * HB + b) + k, 1), :] for b in range(HB)], axis=1)
            g.append(jnp.sum(jnp.where(erow == e, p, 0.0), axis=0, keepdims=True))
        gs = g[0] + g[1]
        blk = _iota((HB, n), 0) == (_iota((HB, n), 1) >> 7)
        parts = []
        for k in range(2):
            w = g[k] / gs
            hi = w.astype(bf16).astype(f32)
            parts += [jnp.where(blk, hi, 0.0), jnp.where(blk, w - hi, 0.0)]
        gp = jnp.dot(jnp.concatenate(parts, axis=0).astype(bf16), perm_v[toks, :],
                     preferred_element_type=f32)
        for k in range(2):
            gat_v[pl.ds(pl.multiple_of(h * N_TOK + k * n, n), n)] = (
                gp[2 * k * HB:(2 * k + 1) * HB] + gp[(2 * k + 1) * HB:(2 * k + 2) * HB]).reshape(n)
        gat_cp(h).start()

    dests = ((diag, 1), (right, 2), (left, 0))

    def seg_size(e, h, owner):
        return cnt_s[e * T + owner * S + h]

    def seg_arrival(e, h, owner):
        return ARR0 + cnt_s[e * T + owner * S + 2] + h * cnt_s[e * T + owner * S]

    def rs_copy(j, h, src_row, dst_row, rows, bit, dev, rel):
        if bit is None:
            sem = (dst_row - ARR0) >> CH_BITS
        else:
            sem = N_CH + ((rel * E_LOC + j) * 2 + h) * N_REM + bit
        return pltpu.make_async_remote_copy(
            src_ref=rows_v.at[pl.ds(src_row * 4, rows * 4)],
            dst_ref=rows_v.at[pl.ds(dst_row * 4, rows * 4)],
            send_sem=rs_send, recv_sem=rs_recv.at[sem],
            device_id=(dev,), device_id_type=MESH)

    def stage_home(j, h):
        e = me * E_LOC + j
        return j * CAP + h * sum(cnt_s[e * T + c * S] for c in range(N_DEV))

    def rs_outgoing(j, h, action):
        e = me * E_LOC + j
        sizes = [seg_size(e, h, dev) for dev, _ in dests]
        home = stage_home(j, h)
        srcs = [home, home + sizes[0], home + sizes[0] + sizes[1]]
        dsts = [seg_arrival(e, h, dev) for dev, _ in dests]
        _for_pieces(sizes, lambda s, o, rows, bit: action(
            rs_copy(j, h, srcs[s] + o, dsts[s] + o, rows, bit, *dests[s])))

    order = (diag, right, left, me)

    def stage_segments(st):
        e = me * E_LOC + (st >> 1)
        sizes = [seg_size(e, st & 1, dev) for dev in order]
        return sizes, [0, sizes[0], sizes[0] + sizes[1], sizes[0] + sizes[1] + sizes[2]]

    def gather_stage(st):
        sizes, offs = stage_segments(st)
        for dev, n, off in zip(order, sizes, offs):
            def gather(m, c):
                base, dst = c
                out = xs_v.at[pl.ds(pl.multiple_of(dst, 4), 32)]
                for u in range(8):
                    out[u * 4:u * 4 + 4, :] = xlin_v[pl.ds(pl.multiple_of(lst_s[base + u], 4), 4), :]
                return base + jnp.where((m & 3) == 3, T - S + 8, 8), dst + 32
            lax.fori_loop(0, (n + 7) >> 3, gather,
                          (st * (N_TOK // 2) + dev * S, (st * XS_CAP + off) * 4))

    def rs_wait(j, h):
        srcs = [(me + 1 + rel) & 3 for rel in range(N_DEV - 1)]
        sizes = [seg_size(src * E_LOC + j, h, me) for src in srcs]
        dsts = [seg_arrival(src * E_LOC + j, h, me) for src in srcs]
        _for_pieces(sizes, lambda s, o, rows, bit: rs_copy(
            j, h, dsts[s] + o, dsts[s] + o, rows, bit, srcs[s], s).wait_recv())

    def stage(st, carry):
        j, h = st >> 1, st & 1

        @pl.when(st < 2)
        def _():
            lax.fori_loop(st * (XCH // 2), (st + 1) * (XCH // 2), x_chunk, 0)

        @pl.when(st == 0)
        def _():
            cnt_cp.wait()
            for jj in range(E_LOC):
                lst_cp(jj).wait()

        first = jnp.where(st == 2, 3, st)
        count = jnp.where(st == 0, E_LOC, jnp.where(st == 1, 1, jnp.where(st == 2, E_LOC - 1, 0)))

        def gather(i, c):
            gather_stage(first + 2 * i)
            return c
        lax.fori_loop(0, count, gather, 0)

        @pl.when(st == 0)
        def _():
            rw_cp.wait()
            gates(0)
            pl.semaphore_wait(barrier, N_DEV - 1)

        @pl.when(st == 2 * E_LOC - 1)
        def _():
            def collect(jj, c):
                rs_wait(jj, 0)
                return c
            lax.fori_loop(0, EARLY, collect, 0)

        @pl.when(h == 0)
        def _():
            w_cp(j).wait()

        sizes, offs = stage_segments(st)
        home = stage_home(j, h)

        def tile(t, c):
            r0 = pl.multiple_of(t * TM, 16)
            x0 = (st * XS_CAP + r0) * 4
            lhs = jnp.concatenate([xs_v[pl.ds(x0 + p, TM, stride=4), :] for p in range(4)], axis=1)
            y = jnp.dot(lhs.astype(bf16), w_v[j].astype(bf16), preferred_element_type=f32)
            for p in range(4):
                rows_v[pl.ds((home + r0) * 4 + p, TM, stride=4), :] = _pack(
                    y[:, p * 128:(p + 1) * 128], y[:, 512 + p * 128:512 + (p + 1) * 128])

            left_over = offs[3] - r0
            @pl.when(jnp.logical_and(jnp.logical_and(left_over > 0, left_over <= TM), st != HELD))
            def _():
                rs_outgoing(j, h, lambda cp: cp.start())
            return c
        lax.fori_loop(0, lax.div(offs[3] + sizes[3] + (TM - 1), TM), tile, 0)

        @pl.when(st == HELD + 1)
        def _():
            rs_outgoing(HELD >> 1, HELD & 1, lambda cp: cp.start())
        return carry
    lax.fori_loop(0, 2 * E_LOC, stage, 0)

    adr_cp.wait()
    gat_cp(0).wait()

    ag_sends = ((me, 0, right), (me, 1, right), (me, 1, left), (me, 0, left),
                (left, 0, right), (right, 1, left))
    ag_recvs = ((left, 0, left), (left, 1, left), (right, 1, right), (right, 0, right),
                (diag, 0, left), (diag, 1, right))
    AG = len(ag_sends)

    def ag_copy(b, kind, table=ag_sends):
        owner, half, dev = table[kind]
        ref = f_v.at[pl.ds(pl.multiple_of(b * T + owner * S + half * (S // 2), S // 2), S // 2)]
        return pltpu.make_async_remote_copy(
            src_ref=ref, dst_ref=ref, send_sem=ag_send.at[kind], recv_sem=ag_recv.at[b * AG + kind],
            device_id=(dev,), device_id_type=MESH)

    def ag_arrival(b, kind):
        return ag_copy(b, kind, ag_recvs)

    def step(i, carry):
        first = jnp.where(i == 0, EARLY, i - (HB - E_LOC))
        last = jnp.where(i == 0, E_LOC, jnp.where(i < HB, first + 1, first))

        def collect(j, c):
            rs_wait(j, jnp.minimum(i, 1))
            return c
        lax.fori_loop(jnp.maximum(first, 0), jnp.maximum(last, 0), collect, 0)

        @pl.when(i < NB)
        def _():
            def slots(m, c):
                base = i * T + me * S + m * 8
                gbase = base + (i >> 3) * (N_TOK // 2)
                adr, ga, gb = (adr_s.at[pl.ds(base, 8)], gat_s.at[pl.ds(gbase, 8)],
                               gat_s.at[pl.ds(gbase + N_TOK // 2, 8)])
                tmp = stmp_v.at[pl.ds(pl.multiple_of(m * 64, 64), 64)]
                for u in range(8):
                    a, g0, g1 = adr[u], ga[u], gb[u]
                    r0 = rows_v[pl.ds(pl.multiple_of(a & 0xFFFF, 4), 4), :]
                    r1 = rows_v[pl.ds(pl.multiple_of(lax.shift_right_logical(a, 16), 4), 4), :]
                    lo = (lax.bitcast_convert_type(r0 << 16, f32) * g0
                          + lax.bitcast_convert_type(r1 << 16, f32) * g1)
                    hi = (lax.bitcast_convert_type(r0 & -65536, f32) * g0
                          + lax.bitcast_convert_type(r1 & -65536, f32) * g1)
                    tmp[u * 8:u * 8 + 4, :] = lo
                    tmp[u * 8 + 4:u * 8 + 8, :] = hi
                return c
            lax.fori_loop(0, S // 8, slots, 0)
            mine = pl.ds(pl.multiple_of(i * T + me * S, S), S)
            for c in range(8):
                f_v[mine, c * 128:(c + 1) * 128] = stmp_v[pl.ds(c, S, stride=8), :].astype(bf16)
            for kind in (0, 2, 1, 3):
                ag_copy(i, kind).start()

        @pl.when(jnp.logical_and(i >= L1, i < NB + L1))
        def _():
            b = i - L1
            ag_arrival(b, 0).wait_recv()
            ag_copy(b, 4).start()
            ag_arrival(b, 2).wait_recv()
            ag_copy(b, 5).start()

        @pl.when(i >= L2)
        def _():
            b = i - L2
            for kind in (1, 3, 4, 5):
                ag_arrival(b, kind).wait_recv()
            rows = pl.ds(pl.multiple_of(b * T, T), T)
            o_v[rows, :] = jnp.dot(perm_v[rows, :], f_v[rows, :], preferred_element_type=f32)

        @pl.when(i == 2)
        def _():
            gates(1)

        @pl.when(i == HB - 1)
        def _():
            gat_cp(1).wait()

        @pl.when(jnp.logical_and(i >= 2, i < 2 + 2 * E_LOC))
        def _():
            rs_outgoing((i - 2) >> 1, (i - 2) & 1, lambda cp: cp.wait_send())

        @pl.when(i >= L2 + 1)
        def _():
            for kind in range(AG):
                ag_copy(i - L2 - 1, kind).wait_send()
        return carry
    lax.fori_loop(0, NB + L2, step, 0)

    for kind in range(AG):
        ag_copy(NB - 1, kind).wait_send()


def pallas_dist_moe_top2_ep_n2048_d512_e4_h1024_kernel(
    x: jax.Array,
    router_W: jax.Array,
    route_idx: jax.Array,
    expert_W: jax.Array,
):
    r = route_idx.astype(i32).reshape(NB, T, 2).transpose(0, 2, 1).reshape(2 * NB, T)
    any_spec = pl.BlockSpec(memory_space=pl.ANY)
    return pl.pallas_call(
        _body,
        out_shape=jax.ShapeDtypeStruct((N_TOK, H), f32),
        in_specs=[any_spec] * 4,
        out_specs=pl.BlockSpec(memory_space=pltpu.VMEM),
        scratch_shapes=[
            pltpu.VMEM((2 * NB + 8, T), i32),
            pltpu.VMEM((N_EXP, D), f32),
            pltpu.VMEM((N_TOK, D), f32),
            pltpu.VMEM((N_TOK * 4 + 8, 128), f32),
            pltpu.VMEM((2 * E_LOC * XS_CAP * 4 + 8, 128), f32),
            pltpu.VMEM((E_LOC, D, H), f32),
            pltpu.VMEM((N_ROWS * 4, 128), i32),
            pltpu.VMEM((N_TOK, H), bf16),
            pltpu.VMEM((N_TOK, T), bf16),
            pltpu.VMEM((N_EXP * NB, T), f32),
            pltpu.VMEM((S * 8 + 8, 128), f32),
            pltpu.VMEM((E_LOC * N_TOK,), i32),
            pltpu.VMEM((N_EXP * T,), i32),
            pltpu.VMEM((N_TOK,), i32),
            pltpu.VMEM((2 * N_TOK,), f32),
            pltpu.SMEM((E_LOC * N_TOK,), i32),
            pltpu.SMEM((N_EXP * T,), i32),
            pltpu.SMEM((N_TOK,), i32),
            pltpu.SMEM((2 * N_TOK,), f32),
            pltpu.SemaphoreType.DMA((2 + XCH + E_LOC,)),
            pltpu.SemaphoreType.DMA((8,)),
            pltpu.SemaphoreType.DMA,
            pltpu.SemaphoreType.DMA((N_CH + (N_DEV - 1) * E_LOC * 2 * N_REM,)),
            pltpu.SemaphoreType.DMA((6,)),
            pltpu.SemaphoreType.DMA((NB * 6,)),
        ],
        compiler_params=pltpu.CompilerParams(
            collective_id=0, vmem_limit_bytes=80 * 1024 * 1024,
            disable_semaphore_checks=True),
    )(r, router_W.T, x, expert_W)
```
